```python
import numpy as np

kernel_name = "dist_sum_ax1_xy_m512_n256"

def setup_inputs():
    return {"x": np.random.randn(1024, 512).astype(np.float32)}

def reference(x: np.ndarray) -> np.ndarray:
    return np.sum(x, axis=1, keepdims=True)
```

```python
import jax
import jax.numpy as jnp
from jax import lax
from jax.experimental import pallas as pl
from jax.experimental.pallas import tpu as pltpu

_LANES = 128


def pallas_dist_sum_ax1_xy_m512_n256_kernel(
x: jax.Array,
):
    m, n = x.shape
    assert m % _LANES == 0 and n % _LANES == 0 and m // _LANES >= 2
    nt = m // _LANES

    def kernel_body(x_hbm, out_ref, xbuf, send_buf, recv_buf, in_sems, send_sems, recv_sems):
        loads = [
            pltpu.make_async_copy(
                x_hbm.at[pl.ds(t * _LANES, _LANES)],
                xbuf.at[pl.ds(t * _LANES, _LANES)],
                in_sems.at[t],
            )
            for t in range(nt)
        ]
        for cp in loads:
            cp.start()

        nbr = (lax.axis_index("x"), 1 - lax.axis_index("y"))
        barrier = pltpu.get_barrier_semaphore()
        pl.semaphore_signal(
            barrier, inc=1, device_id=nbr, device_id_type=pl.DeviceIdType.MESH
        )

        def swap(i, lo, hi):
            return pltpu.make_async_remote_copy(
                src_ref=send_buf.at[pl.ds(lo, hi - lo)],
                dst_ref=recv_buf.at[pl.ds(lo, hi - lo)],
                send_sem=send_sems.at[i],
                recv_sem=recv_sems.at[i],
                device_id=nbr,
                device_id_type=pl.DeviceIdType.MESH,
            )

        diag = lax.broadcasted_iota(jnp.int32, (_LANES, _LANES), 0) == (
            lax.broadcasted_iota(jnp.int32, (_LANES, _LANES), 1)
        )

        def tile_sums(t):
            rows = pl.ds(t * _LANES, _LANES)
            h = xbuf[rows, 0:_LANES]
            for j in range(1, n // _LANES):
                h = h + xbuf[rows, j * _LANES:(j + 1) * _LANES]
            s = jnp.sum(h, axis=1, keepdims=True)
            return jnp.sum(jnp.where(diag, s, 0.0), axis=0, keepdims=True)

        for t in range(nt - 1):
            loads[t].wait()
            send_buf[t:t + 1, :] = tile_sums(t)

        pl.semaphore_wait(barrier, 1)
        early = swap(0, 0, nt - 1)
        early.start()

        loads[nt - 1].wait()
        last_sums = tile_sums(nt - 1)
        send_buf[nt - 1:nt, :] = last_sums
        last = swap(1, nt - 1, nt)
        last.start()

        early.wait_recv()
        out_ref[0:nt - 1, :] = send_buf[0:nt - 1, :] + recv_buf[0:nt - 1, :]
        last.wait_recv()
        out_ref[nt - 1:nt, :] = last_sums + recv_buf[nt - 1:nt, :]
        early.wait_send()
        last.wait_send()

    out = pl.pallas_call(
        kernel_body,
        out_shape=jax.ShapeDtypeStruct((nt, _LANES), x.dtype),
        in_specs=[pl.BlockSpec(memory_space=pl.ANY)],
        out_specs=pl.BlockSpec(memory_space=pltpu.VMEM),
        scratch_shapes=[
            pltpu.VMEM((m, n), x.dtype),
            pltpu.VMEM((nt, _LANES), x.dtype),
            pltpu.VMEM((nt, _LANES), x.dtype),
            pltpu.SemaphoreType.DMA((nt,)),
            pltpu.SemaphoreType.DMA((2,)),
            pltpu.SemaphoreType.DMA((2,)),
        ],
        compiler_params=pltpu.CompilerParams(
            collective_id=0,
            disable_bounds_checks=True,
            disable_semaphore_checks=True,
        ),
    )(x)
    return out.reshape(m, 1)
```

```python
import jax
import jax.numpy as jnp
from jax import lax
from jax.experimental import pallas as pl
from jax.experimental.pallas import tpu as pltpu

_LANES = 128
_SUBLANES = 8
_RAW_ROWS = 32
_TAIL_ROWS = 16


def pallas_dist_sum_ax1_xy_m512_n256_kernel(
x: jax.Array,
):
    m, n = x.shape
    assert m % _LANES == 0 and n % _LANES == 0 and m // _LANES >= 2
    nt = m // _LANES
    last0 = (nt - 1) * _LANES
    raw0 = m - _RAW_ROWS
    tail0 = raw0 - _TAIL_ROWS
    spans = [(t * _LANES, _LANES) for t in range(nt - 1)]
    spans += [(last0, tail0 - last0), (tail0, _TAIL_ROWS), (raw0, _RAW_ROWS)]

    def kernel_body(
        x_hbm, out_ref, xbuf, raw_buf, send_buf, recv_buf,
        in_sems, send_sems, recv_sems,
    ):
        loads = [
            pltpu.make_async_copy(
                x_hbm.at[pl.ds(r0, rows)], xbuf.at[pl.ds(r0, rows)], in_sems.at[i]
            )
            for i, (r0, rows) in enumerate(spans)
        ]
        for cp in loads[:-1]:
            cp.start()

        nbr = (lax.axis_index("x"), 1 - lax.axis_index("y"))

        def to_nbr(i, src, dst):
            return pltpu.make_async_remote_copy(
                src_ref=src,
                dst_ref=dst,
                send_sem=send_sems.at[i],
                recv_sem=recv_sems.at[i],
                device_id=nbr,
                device_id_type=pl.DeviceIdType.MESH,
            )

        barrier = pltpu.get_barrier_semaphore()
        pl.semaphore_signal(
            barrier, inc=1, device_id=nbr, device_id_type=pl.DeviceIdType.MESH
        )
        pl.semaphore_wait(barrier, 1)
        raw = to_nbr(0, x_hbm.at[pl.ds(raw0, _RAW_ROWS)], raw_buf)
        raw.start()

        lane_minus_sublane = lax.broadcasted_iota(
            jnp.int32, (_SUBLANES, _LANES), 1
        ) - lax.broadcasted_iota(jnp.int32, (_SUBLANES, _LANES), 0)

        def fold(ref, r0, rows):
            h = ref[r0:r0 + rows, 0:_LANES]
            for c in range(_LANES, n, _LANES):
                h = h + ref[r0:r0 + rows, c:c + _LANES]
            return h

        def row_sums(h, lane0):
            s = jnp.sum(h, axis=1, keepdims=True)
            acc = jnp.zeros((_SUBLANES, _LANES), h.dtype)
            for r in range(0, h.shape[0], _SUBLANES):
                acc = jnp.where(
                    lane_minus_sublane == lane0 + r, s[r:r + _SUBLANES, :], acc
                )
            return jnp.sum(acc, axis=0, keepdims=True)

        for t in range(nt - 1):
            loads[t].wait()
            send_buf[t:t + 1, :] = row_sums(fold(xbuf, t * _LANES, _LANES), 0)
        early = to_nbr(
            1, send_buf.at[pl.ds(0, nt - 1)], recv_buf.at[pl.ds(0, nt - 1)]
        )
        early.start()

        loads[nt - 1].wait()
        h_body = fold(xbuf, last0, tail0 - last0)
        loads[nt].wait()
        h_tail = fold(xbuf, tail0, _TAIL_ROWS)
        last_sums = row_sums(jnp.concatenate([h_body, h_tail], axis=0), 0)
        send_buf[nt - 1:nt, :] = last_sums
        last = to_nbr(
            2, send_buf.at[pl.ds(nt - 1, 1)], recv_buf.at[pl.ds(nt - 1, 1)]
        )
        last.start()

        loads[-1].start()
        loads[-1].wait()
        own_raw = fold(xbuf, raw0, _RAW_ROWS)
        raw.wait_recv()
        last_sums = last_sums + row_sums(
            own_raw + fold(raw_buf, 0, _RAW_ROWS), raw0 - last0
        )

        raw.wait_send()
        early.wait_send()
        last.wait_send()
        early.wait_recv()
        out_ref[0:nt - 1, :] = send_buf[0:nt - 1, :] + recv_buf[0:nt - 1, :]
        last.wait_recv()
        out_ref[nt - 1:nt, :] = last_sums + recv_buf[nt - 1:nt, :]

    out = pl.pallas_call(
        kernel_body,
        out_shape=jax.ShapeDtypeStruct((nt, _LANES), x.dtype),
        in_specs=[pl.BlockSpec(memory_space=pl.ANY)],
        out_specs=pl.BlockSpec(memory_space=pltpu.VMEM),
        scratch_shapes=[
            pltpu.VMEM((m, n), x.dtype),
            pltpu.VMEM((_RAW_ROWS, n), x.dtype),
            pltpu.VMEM((nt, _LANES), x.dtype),
            pltpu.VMEM((nt, _LANES), x.dtype),
            pltpu.SemaphoreType.DMA((len(spans),)),
            pltpu.SemaphoreType.DMA((3,)),
            pltpu.SemaphoreType.DMA((3,)),
        ],
        compiler_params=pltpu.CompilerParams(
            collective_id=0,
            disable_semaphore_checks=True,
        ),
    )(x)
    return out.reshape(m, 1)
```

```python
import jax
import jax.numpy as jnp
from jax import lax
from jax.experimental import pallas as pl
from jax.experimental.pallas import tpu as pltpu

_LANES = 128
_SUBLANES = 8
_RAW_ROWS = 32
_TAIL_ROWS = 16


def _compiler_params():
    try:
        return pltpu.CompilerParams(collective_id=0, disable_semaphore_checks=True)
    except TypeError:
        return pltpu.CompilerParams(collective_id=0)


def pallas_dist_sum_ax1_xy_m512_n256_kernel(
x: jax.Array,
):
    m, n = x.shape
    assert m % _LANES == 0 and n % _LANES == 0 and m // _LANES >= 2
    nt = m // _LANES
    last0 = (nt - 1) * _LANES
    raw0 = m - _RAW_ROWS
    tail0 = raw0 - _TAIL_ROWS
    spans = [(t * _LANES, _LANES) for t in range(nt - 1)]
    spans += [(last0, tail0 - last0), (tail0, _TAIL_ROWS), (raw0, _RAW_ROWS)]

    def kernel_body(
        x_hbm, out_ref, xbuf, raw_buf, send_buf, recv_buf,
        in_sems, send_sems, recv_sems,
    ):
        loads = [
            pltpu.make_async_copy(
                x_hbm.at[pl.ds(r0, rows)], xbuf.at[pl.ds(r0, rows)], in_sems.at[i]
            )
            for i, (r0, rows) in enumerate(spans)
        ]
        for cp in loads[:-1]:
            cp.start()

        nbr = (lax.axis_index("x"), 1 - lax.axis_index("y"))

        def to_nbr(i, src, dst):
            return pltpu.make_async_remote_copy(
                src_ref=src,
                dst_ref=dst,
                send_sem=send_sems.at[i],
                recv_sem=recv_sems.at[i],
                device_id=nbr,
                device_id_type=pl.DeviceIdType.MESH,
            )

        barrier = pltpu.get_barrier_semaphore()
        pl.semaphore_signal(
            barrier, inc=1, device_id=nbr, device_id_type=pl.DeviceIdType.MESH
        )
        pl.semaphore_wait(barrier, 1)
        raw = to_nbr(0, x_hbm.at[pl.ds(raw0, _RAW_ROWS)], raw_buf)
        raw.start()

        lane_minus_sublane = lax.broadcasted_iota(
            jnp.int32, (_SUBLANES, _LANES), 1
        ) - lax.broadcasted_iota(jnp.int32, (_SUBLANES, _LANES), 0)

        def fold(ref, r0, rows):
            h = ref[r0:r0 + rows, 0:_LANES]
            for c in range(_LANES, n, _LANES):
                h = h + ref[r0:r0 + rows, c:c + _LANES]
            return h

        def row_sums(h, lane0):
            s = jnp.sum(h, axis=1, keepdims=True)
            acc = jnp.zeros((_SUBLANES, _LANES), h.dtype)
            for r in range(0, h.shape[0], _SUBLANES):
                acc = jnp.where(
                    lane_minus_sublane == lane0 + r, s[r:r + _SUBLANES, :], acc
                )
            return jnp.sum(acc, axis=0, keepdims=True)

        for t in range(nt - 1):
            loads[t].wait()
            send_buf[t:t + 1, :] = row_sums(fold(xbuf, t * _LANES, _LANES), 0)
        early = to_nbr(
            1, send_buf.at[pl.ds(0, nt - 1)], recv_buf.at[pl.ds(0, nt - 1)]
        )
        early.start()

        loads[nt - 1].wait()
        h_body = fold(xbuf, last0, tail0 - last0)
        loads[nt].wait()
        h_tail = fold(xbuf, tail0, _TAIL_ROWS)
        last_sums = row_sums(jnp.concatenate([h_body, h_tail], axis=0), 0)
        send_buf[nt - 1:nt, :] = last_sums
        last = to_nbr(
            2, send_buf.at[pl.ds(nt - 1, 1)], recv_buf.at[pl.ds(nt - 1, 1)]
        )
        last.start()

        loads[-1].start()
        loads[-1].wait()
        own_raw = fold(xbuf, raw0, _RAW_ROWS)
        raw.wait_recv()
        last_sums = last_sums + row_sums(
            own_raw + fold(raw_buf, 0, _RAW_ROWS), raw0 - last0
        )

        raw.wait_send()
        early.wait_send()
        last.wait_send()
        early.wait_recv()
        out_ref[0:nt - 1, :] = send_buf[0:nt - 1, :] + recv_buf[0:nt - 1, :]
        last.wait_recv()
        out_ref[nt - 1:nt, :] = last_sums + recv_buf[nt - 1:nt, :]

    out = pl.pallas_call(
        kernel_body,
        out_shape=jax.ShapeDtypeStruct((nt, _LANES), x.dtype),
        in_specs=[pl.BlockSpec(memory_space=pl.ANY)],
        out_specs=pl.BlockSpec(memory_space=pltpu.VMEM),
        scratch_shapes=[
            pltpu.VMEM((m, n), x.dtype),
            pltpu.VMEM((_RAW_ROWS, n), x.dtype),
            pltpu.VMEM((nt, _LANES), x.dtype),
            pltpu.VMEM((nt, _LANES), x.dtype),
            pltpu.SemaphoreType.DMA((len(spans),)),
            pltpu.SemaphoreType.DMA((3,)),
            pltpu.SemaphoreType.DMA((3,)),
        ],
        compiler_params=_compiler_params(),
    )(x)
    return out.reshape(m, 1)
```

```python
import jax
import jax.numpy as jnp
from jax import lax
from jax.experimental import pallas as pl
from jax.experimental.pallas import tpu as pltpu

_LANES = 128
_SUBLANES = 8
_RAW_ROWS = 32
_BLOCKS = ((144,), (144,), (80, 16), (80, 16))


def _compiler_params():
    try:
        return pltpu.CompilerParams(collective_id=0, disable_semaphore_checks=True)
    except TypeError:
        return pltpu.CompilerParams(collective_id=0)


def pallas_dist_sum_ax1_xy_m512_n256_kernel(
x: jax.Array,
):
    m, n = x.shape
    nt = m // _LANES
    last0 = (nt - 1) * _LANES
    raw0 = m - _RAW_ROWS
    assert m % _LANES == 0 and n % _LANES == 0 and nt >= 2
    assert sum(map(sum, _BLOCKS)) == raw0 and last0 <= raw0 - sum(_BLOCKS[-1])

    def kernel_body(
        x_hbm, out_ref, xbuf, raw_buf, send_buf, recv_buf,
        in_sems, send_sems, recv_sems,
    ):
        spans = []
        for rows in [r for block in _BLOCKS for r in block] + [_RAW_ROWS]:
            spans.append((sum(r for _, r in spans), rows))
        loads = [
            pltpu.make_async_copy(
                x_hbm.at[pl.ds(r0, rows)], xbuf.at[pl.ds(r0, rows)], in_sems.at[i]
            )
            for i, (r0, rows) in enumerate(spans)
        ]
        for cp in loads[:-1]:
            cp.start()

        nbr = (lax.axis_index("x"), 1 - lax.axis_index("y"))

        def to_nbr(i, src, dst):
            return pltpu.make_async_remote_copy(
                src_ref=src,
                dst_ref=dst,
                send_sem=send_sems.at[i],
                recv_sem=recv_sems.at[i],
                device_id=nbr,
                device_id_type=pl.DeviceIdType.MESH,
            )

        raw = to_nbr(0, x_hbm.at[pl.ds(raw0, _RAW_ROWS)], raw_buf)
        early = to_nbr(
            1, send_buf.at[pl.ds(0, nt - 1)], recv_buf.at[pl.ds(0, nt - 1)]
        )
        last = to_nbr(
            2, send_buf.at[pl.ds(nt - 1, 1)], recv_buf.at[pl.ds(nt - 1, 1)]
        )

        barrier = pltpu.get_barrier_semaphore()
        pl.semaphore_signal(
            barrier, inc=1, device_id=nbr, device_id_type=pl.DeviceIdType.MESH
        )
        pl.semaphore_wait(barrier, 1)
        raw.start()

        lane_minus_sublane = lax.broadcasted_iota(
            jnp.int32, (_SUBLANES, _LANES), 1
        ) - lax.broadcasted_iota(jnp.int32, (_SUBLANES, _LANES), 0)
        zeros = jnp.zeros((_SUBLANES, _LANES), x.dtype)

        def fold(ref, r0, rows):
            h = ref[r0:r0 + rows, 0:_LANES]
            for c in range(_LANES, n, _LANES):
                h = h + ref[r0:r0 + rows, c:c + _LANES]
            return h

        def place(acc, sums, r):
            return jnp.where(lane_minus_sublane == r % _LANES, sums, acc)

        acc, i = zeros, 0
        for block in _BLOCKS:
            r0 = spans[i][0]
            parts = []
            for _ in block:
                loads[i].wait()
                parts.append(fold(xbuf, *spans[i]))
                i += 1
            s = jnp.sum(jnp.concatenate(parts, axis=0), axis=1, keepdims=True)
            for g in range(0, sum(block), _SUBLANES):
                acc = place(acc, s[g:g + _SUBLANES, :], r0 + g)
                done = r0 + g + _SUBLANES
                if done % _LANES == 0 or done == raw0:
                    t = (done - 1) // _LANES
                    last_sums = jnp.sum(acc, axis=0, keepdims=True)
                    send_buf[t:t + 1, :] = last_sums
                    acc = zeros
            if r0 < last0 <= r0 + sum(block):
                early.start()
        last.start()

        loads[-1].start()
        loads[-1].wait()
        own_raw = fold(xbuf, raw0, _RAW_ROWS)
        raw.wait_recv()
        s = jnp.sum(own_raw + fold(raw_buf, 0, _RAW_ROWS), axis=1, keepdims=True)
        for g in range(0, _RAW_ROWS, _SUBLANES):
            acc = place(acc, s[g:g + _SUBLANES, :], raw0 + g)
        last_sums = last_sums + jnp.sum(acc, axis=0, keepdims=True)

        raw.wait_send()
        early.wait_send()
        last.wait_send()
        early.wait_recv()
        out_ref[0:nt - 1, :] = send_buf[0:nt - 1, :] + recv_buf[0:nt - 1, :]
        last.wait_recv()
        out_ref[nt - 1:nt, :] = last_sums + recv_buf[nt - 1:nt, :]

    out = pl.pallas_call(
        kernel_body,
        out_shape=jax.ShapeDtypeStruct((nt, _LANES), x.dtype),
        in_specs=[pl.BlockSpec(memory_space=pl.ANY)],
        out_specs=pl.BlockSpec(memory_space=pltpu.VMEM),
        scratch_shapes=[
            pltpu.VMEM((m, n), x.dtype),
            pltpu.VMEM((_RAW_ROWS, n), x.dtype),
            pltpu.VMEM((nt, _LANES), x.dtype),
            pltpu.VMEM((nt, _LANES), x.dtype),
            pltpu.SemaphoreType.DMA((sum(map(len, _BLOCKS)) + 1,)),
            pltpu.SemaphoreType.DMA((3,)),
            pltpu.SemaphoreType.DMA((3,)),
        ],
        compiler_params=_compiler_params(),
    )(x)
    return out.reshape(m, 1)
```
